```python
import numpy as np

kernel_name = "dist_ring_attn_i_s256_d64"

def setup_inputs():
    S, D = 1024, 64
    q = np.random.randn(S, D).astype(np.float32)
    k = np.random.randn(S, D).astype(np.float32)
    v = np.random.randn(S, D).astype(np.float32)
    return {"q": q, "k": k, "v": v}

def reference(q: np.ndarray, k: np.ndarray, v: np.ndarray) -> np.ndarray:
    D = q.shape[1]
    scores = q @ k.T / np.sqrt(D)
    scores_max = np.max(scores, axis=1, keepdims=True)
    weights = np.exp(scores - scores_max)
    weights = weights / np.sum(weights, axis=1, keepdims=True)
    return weights @ v
```

```python
import jax
import jax.numpy as jnp
from jax import lax
from jax.experimental import pallas as pl
from jax.experimental.pallas import tpu as pltpu

N_DEV = 4
LOG2E = 1.4426950408889634
MESH = pl.DeviceIdType.MESH


def pallas_dist_ring_attn_i_s256_d64_kernel(q, k, v):
    S, D = q.shape
    HK = S // 2
    scale = LOG2E / (D ** 0.5)
    f32, bf16 = jnp.float32, jnp.bfloat16

    def body(q_hbm, k_hbm, v_hbm, o_ref, stage, buf, in_sems, send_sems, recv_sems):
        me = lax.axis_index("i")
        left = lax.rem(me + (N_DEV - 1), N_DEV)
        right = lax.rem(me + 1, N_DEV)

        barrier = pltpu.get_barrier_semaphore()
        pl.semaphore_signal(barrier, 1, device_id=(left,), device_id_type=MESH)
        pl.semaphore_signal(barrier, 1, device_id=(right,), device_id_type=MESH)

        ld_k = pltpu.make_async_copy(k_hbm, stage.at[0], in_sems.at[0])
        ld_v = pltpu.make_async_copy(v_hbm, stage.at[1], in_sems.at[1])
        ld_q = pltpu.make_async_copy(q_hbm, stage.at[2], in_sems.at[2])
        ld_k.start()
        ld_v.start()
        ld_q.start()

        KA, VA, KB, VB = 0, 1, 2, 3

        def rcopy(src_slot, dst_slot, piece, target):
            return pltpu.make_async_remote_copy(
                src_ref=buf.at[src_slot, piece],
                dst_ref=buf.at[dst_slot, piece],
                send_sem=send_sems.at[src_slot * 4 + piece if src_slot else (dst_slot - 1) * 12 + piece],
                recv_sem=recv_sems.at[dst_slot * 4 + piece],
                device_id=(target,),
                device_id_type=MESH,
            )

        to_r = {p: rcopy(0, 1, p, right) for p in range(4)}
        to_l = {p: rcopy(0, 2, p, left) for p in range(4)}
        fw_r = {p: rcopy(1, 3, p, right) for p in (KA, VA)}
        fw_l = {p: rcopy(2, 3, p, left) for p in (KB, VB)}

        ld_k.wait()
        kt = stage[0].astype(bf16)
        k2 = jnp.concatenate([kt[:, :HK], kt[:, HK:]], axis=0).T
        buf[0, KA] = k2[:D]
        buf[0, KB] = k2[D:]

        pl.semaphore_wait(barrier, 2)
        to_r[KA].start()
        to_l[KB].start()

        ld_v.wait()
        vt = stage[1].astype(bf16)
        v_a = jnp.concatenate([vt[:, 0:D], vt[:, HK:HK + D]], axis=1)
        v_b = jnp.concatenate([vt[:, D:HK], vt[:, HK + D:]], axis=1)
        buf[0, VA] = v_a
        buf[0, VB] = v_b
        to_r[VA].start()
        to_l[VB].start()
        to_r[KB].start()
        to_l[KA].start()
        to_r[VB].start()
        to_l[VA].start()

        ld_q.wait()
        qs = (stage[2] * scale).astype(bf16)
        zq = jnp.zeros_like(qs)
        w_top = jnp.concatenate([qs, zq], axis=0)
        w_bot = jnp.concatenate([zq, qs], axis=0)

        def scores(k2_pair):
            s_top = jnp.dot(k2_pair, w_top, preferred_element_type=f32)
            s_bot = jnp.dot(k2_pair, w_bot, preferred_element_type=f32)
            return jnp.concatenate([s_top[:D], s_bot[:D], s_top[D:], s_bot[D:]], axis=0)

        def softmax_step(s, state):
            m_blk = jnp.max(s, axis=0, keepdims=True)
            if state is None:
                m_new = m_blk
            else:
                m_new = jnp.maximum(state[0], m_blk)
            p = jnp.exp2(s - m_new)
            l_blk = jnp.sum(p, axis=0, keepdims=True)
            return p.astype(bf16), m_new, l_blk

        def accumulate(p, m_new, l_blk, vt_pair, state):
            pv = jnp.dot(vt_pair, p, preferred_element_type=f32)
            if state is None:
                return m_new, l_blk, pv
            m_old, l_old, acc = state
            alpha = jnp.exp2(m_old - m_new)
            return m_new, l_old * alpha + l_blk, acc * alpha + pv

        p, m, l = softmax_step(scores(k2), None)
        st = accumulate(p, m, l, jnp.concatenate([v_a, v_b], axis=1), None)

        to_r[KA].wait_recv(); fw_r[KA].start()
        to_l[KB].wait_recv(); fw_l[KB].start()
        to_r[VA].wait_recv(); fw_r[VA].start()
        to_l[VB].wait_recv(); fw_l[VB].start()
        p, m, l = softmax_step(scores(jnp.concatenate([buf[1, KA], buf[2, KB]], axis=0)), st)
        st = accumulate(p, m, l, jnp.concatenate([buf[1, VA], buf[2, VB]], axis=1), st)

        to_r[KB].wait_recv()
        to_l[KA].wait_recv()
        p, m, l = softmax_step(scores(jnp.concatenate([buf[1, KB], buf[2, KA]], axis=0)), st)
        to_r[VB].wait_recv()
        to_l[VA].wait_recv()
        st = accumulate(p, m, l, jnp.concatenate([buf[1, VB], buf[2, VA]], axis=1), st)
        for p_ in range(4):
            to_r[p_].wait_send()
            to_l[p_].wait_send()

        fw_r[KA].wait_recv()
        fw_l[KB].wait_recv()
        p, m, l = softmax_step(scores(jnp.concatenate([buf[3, KA], buf[3, KB]], axis=0)), st)
        for c in (fw_r[KA], fw_l[KB], fw_r[VA], fw_l[VB]):
            c.wait_send()
        fw_r[VA].wait_recv()
        fw_l[VB].wait_recv()
        m, l, acc = accumulate(p, m, l, jnp.concatenate([buf[3, VA], buf[3, VB]], axis=1), st)
        o_ref[...] = acc * pl.reciprocal(l, approx=False)

    out_t = pl.pallas_call(
        body,
        out_shape=jax.ShapeDtypeStruct((D, S), f32),
        in_specs=[pl.BlockSpec(memory_space=pl.ANY)] * 3,
        out_specs=pl.BlockSpec(memory_space=pltpu.VMEM),
        scratch_shapes=[
            pltpu.VMEM((3, D, S), f32),
            pltpu.VMEM((4, 4, D, 2 * D), bf16),
            pltpu.SemaphoreType.DMA((3,)),
            pltpu.SemaphoreType.DMA((16,)),
            pltpu.SemaphoreType.DMA((16,)),
        ],
        compiler_params=pltpu.CompilerParams(collective_id=0, disable_semaphore_checks=True),
    )(q.T, k.T, v.T)
    return out_t.T
```

```python
import jax
import jax.numpy as jnp
from jax import lax
from jax.experimental import pallas as pl
from jax.experimental.pallas import tpu as pltpu

N_DEV = 4
LOG2E = 1.4426950408889634
MESH = pl.DeviceIdType.MESH
FIRST, NEAR_R, LAST, NEAR_L = 0, 1, 2, 3
KA, VA, KB, VB = 0, 1, 2, 3
NCH = 4
NF32 = 2
DIRECT = ((KB, 0), (KB, 1), (KB, 2), (KB, 3), (VB, 0), (VB, 1), (VB, 2), (VB, 3), (KA, 3), (VA, 3))
SAFE_EXP = 40.0


def pallas_dist_ring_attn_i_s256_d64_kernel(q, k, v):
    S, D = q.shape
    HK = S // 2
    R = D // NCH
    scale = LOG2E / (D ** 0.5)
    f32, bf16 = jnp.float32, jnp.bfloat16
    NT = (((1,), (1,)), ((), ()))
    chunks = range(NCH)

    def body(q_hbm, k_hbm, v_hbm, o_ref, stage, buf, fbuf, in_sems, send_sems, recv_sems, ready, dsend):
        me = lax.axis_index("i")
        left = (me + (N_DEV - 1)) & (N_DEV - 1)
        right = (me + 1) & (N_DEV - 1)
        near = (me & 1) == 1
        barrier = pltpu.get_barrier_semaphore()

        def signal(sem, target):
            pl.semaphore_signal(sem, 1, device_id=(target,), device_id_type=MESH)

        def rows(c):
            return pl.ds(c * R, R)

        ld_k = [pltpu.make_async_copy(k_hbm.at[rows(c)], stage.at[0, rows(c)], in_sems.at[c]) for c in chunks]
        ld_v = [pltpu.make_async_copy(v_hbm.at[rows(c)], stage.at[1, rows(c)], in_sems.at[NCH + c]) for c in chunks]
        ld_q = pltpu.make_async_copy(q_hbm, stage.at[2], in_sems.at[2 * NCH])

        @pl.when(near)
        def _():
            signal(barrier, LAST)

        for cp in ld_k + ld_v + [ld_q]:
            cp.start()

        @pl.when(me == FIRST)
        def _():
            signal(barrier, NEAR_R)
            signal(barrier, NEAR_L)
            signal(barrier, LAST)

        def remote(src, dst, send_sem, dst_slot, piece, c, target):
            return pltpu.make_async_remote_copy(
                src_ref=src, dst_ref=dst, send_sem=send_sem,
                recv_sem=recv_sems.at[((dst_slot - 1) * 4 + piece) * NCH + c],
                device_id=(target,), device_id_type=MESH)

        def own(dst_slot, piece, c, target):
            send_sem = send_sems.at[((dst_slot - 1) * 4 + piece) * NCH + c]
            if (dst_slot, piece) in ((1, KA), (2, KB)) and c < NF32:
                return remote(k_hbm.at[rows(c), pl.ds((piece // 2) * HK, HK)], fbuf.at[dst_slot - 1, c],
                              send_sem, dst_slot, piece, c, target)
            return remote(buf.at[0, piece, rows(c)], buf.at[dst_slot, piece, rows(c)],
                          send_sem, dst_slot, piece, c, target)

        def relay(src_slot, piece, c, target):
            return remote(buf.at[src_slot, piece, rows(c)], buf.at[3, piece, rows(c)],
                          send_sems.at[(8 + piece) * NCH + c], 3, piece, c, target)

        to_r = {(p, c): own(1, p, c, right) for p in range(4) for c in chunks}
        to_l = {(p, c): own(2, p, c, left) for p in range(4) for c in chunks}
        fw = {(p, c): relay(1, p, c, right) for p in (KA, VA) for c in chunks}
        fw.update({(p, c): relay(2, p, c, left) for p in (KB, VB) for c in chunks})
        direct = {(p, c): remote(buf.at[0, p, rows(c)], buf.at[3, p, rows(c)], dsend.at[p * NCH + c],
                                 3, p, c, FIRST) for p, c in DIRECT}

        def start_if(cond, cp):
            @pl.when(cond)
            def _():
                cp.start()

        @pl.when(me == LAST)
        def _():
            pl.semaphore_wait(barrier, 3)
            for c in range(NF32):
                to_r[KA, c].start()
            to_l[KB, 0].start()
            signal(ready, NEAR_R)
            signal(ready, NEAR_L)

        @pl.when(near)
        def _():
            pl.semaphore_wait(barrier, 1)
            signal(ready, FIRST)

        early_r = (me == LAST) | (me == NEAR_L)
        early_l = (me == LAST) | (me == NEAR_R)

        @pl.when(me == NEAR_L)
        def _():
            for c in range(NF32):
                to_r[KA, c].start()

        @pl.when(me == NEAR_R)
        def _():
            for c in range(NF32):
                to_l[KB, c].start()

        k_parts, v_parts = [], []
        for c in chunks:
            ld_k[c].wait()
            kc = stage[0, rows(c)].astype(bf16)
            k_parts.append(kc)
            buf[0, KA, rows(c)] = kc[:, :HK]
            buf[0, KB, rows(c)] = kc[:, HK:]
            for p in (KB, KA):
                if (p, c) in DIRECT:
                    start_if(me == LAST, direct[p, c])
            if c >= NF32:
                start_if(me == NEAR_L if (KA, c) in DIRECT else early_r, to_r[KA, c])
                start_if(me == NEAR_R, to_l[KB, c])
        for c in chunks:
            ld_v[c].wait()
            vc = stage[1, rows(c)].astype(bf16)
            v_parts.append(vc)
            buf[0, VA, rows(c)] = vc[:, :HK]
            buf[0, VB, rows(c)] = vc[:, HK:]
            for p in (VB, VA):
                if (p, c) in DIRECT:
                    start_if(me == LAST, direct[p, c])
            start_if(me == NEAR_L if (VA, c) in DIRECT else early_r, to_r[VA, c])
            start_if(me == NEAR_R, to_l[VB, c])
        kt = jnp.concatenate(k_parts, axis=0)
        vt = jnp.concatenate(v_parts, axis=0)

        @pl.when(me == LAST)
        def _():
            for key in [(p, c) for p in (KA, VA) for c in chunks if (p, c) in DIRECT]:
                to_r[key].start()
            for key in [(KB, c) for c in chunks][1:] + [(VB, c) for c in chunks]:
                to_l[key].start()

        for pr, pl_ in ((KB, KA), (VB, VA)):
            for c in chunks:
                start_if(early_r, to_r[pr, c])
                start_if(early_l, to_l[pl_, c])

        @pl.when(me == FIRST)
        def _():
            pl.semaphore_wait(ready, 2)
            for pr, pl_ in zip((KA, VA, KB, VB), (KB, VB, KA, VA)):
                for c in chunks:
                    to_r[pr, c].start()
                    to_l[pl_, c].start()

        @pl.when(me == NEAR_R)
        def _():
            pl.semaphore_wait(ready, 1)
            for p in (KA, VA, KB, VB):
                for c in chunks:
                    to_r[p, c].start()

        @pl.when(me == NEAR_L)
        def _():
            pl.semaphore_wait(ready, 1)
            for p in (KB, VB, KA, VA):
                for c in chunks:
                    to_l[p, c].start()

        ld_q.wait()
        qb = (stage[2] * scale).astype(bf16).T
        ones = jnp.ones((16, S), bf16)

        def scores(kt_pair):
            return jnp.concatenate(
                [jnp.dot(qb[:HK], kt_pair, preferred_element_type=f32),
                 jnp.dot(qb[HK:], kt_pair, preferred_element_type=f32)], axis=0)

        def weighted(vt_pair, p):
            return lax.dot_general(jnp.concatenate([ones, vt_pair], axis=0), p, NT,
                                   preferred_element_type=f32)

        s = scores(kt)
        m0 = jnp.max(s, axis=1, keepdims=True)
        acc = weighted(vt, jnp.exp2(s - m0).astype(bf16))

        def weights(kt_pair, worst):
            e = scores(kt_pair) - m0
            return jnp.exp2(e).astype(bf16), jnp.maximum(worst, jnp.max(e, axis=0, keepdims=True))

        def relay_left(p, c):
            to_r[p, c].wait_recv()
            if p == KA and c < NF32:
                buf[1, KA, rows(c)] = fbuf[0, c].astype(bf16)
            if (p, c) in DIRECT:
                start_if(me != NEAR_L, fw[p, c])
            else:
                fw[p, c].start()

        def relay_right(p, c):
            to_l[p, c].wait_recv()
            if p == KB and c < NF32:
                buf[2, KB, rows(c)] = fbuf[1, c].astype(bf16)
            if (p, c) in DIRECT:
                start_if(me != NEAR_R, fw[p, c])
            else:
                fw[p, c].start()

        from_l = [(p, c) for p in (KA, VA) for c in chunks]
        from_r = [(p, c) for p in (KB, VB) for c in chunks]

        @pl.when(me == NEAR_L)
        def _():
            for x in [x for x in from_l if x not in DIRECT] + [x for x in from_l if x in DIRECT]:
                relay_left(*x)
            for x in from_r:
                relay_right(*x)

        @pl.when(me == NEAR_R)
        def _():
            for x in from_r:
                relay_right(*x)
            for x in from_l:
                relay_left(*x)

        @pl.when(jnp.logical_not(near))
        def _():
            for x, y in zip(from_l, from_r):
                relay_left(*x)
                relay_right(*y)

        worst = jnp.zeros((1, S), f32)
        p, worst = weights(jnp.concatenate([buf[1, KA], buf[2, KB]], axis=1), worst)
        acc += weighted(jnp.concatenate([buf[1, VA], buf[2, VB]], axis=1), p)

        for c in chunks:
            to_r[KB, c].wait_recv()
            to_l[KA, c].wait_recv()
        p, worst = weights(jnp.concatenate([buf[1, KB], buf[2, KA]], axis=1), worst)
        for c in chunks:
            to_r[VB, c].wait_recv()
            to_l[VA, c].wait_recv()
        acc += weighted(jnp.concatenate([buf[1, VB], buf[2, VA]], axis=1), p)

        for cp in list(to_r.values()) + list(to_l.values()):
            cp.wait_send()
        for key, cp in fw.items():
            if key in DIRECT:
                @pl.when(me != (NEAR_L if key[0] in (KA, VA) else NEAR_R))
                def _():
                    cp.wait_send()
            else:
                cp.wait_send()

        @pl.when(me == LAST)
        def _():
            for cp in direct.values():
                cp.wait_send()

        for c in chunks:
            fw[KA, c].wait_recv()
            fw[KB, c].wait_recv()
        p, worst = weights(jnp.concatenate([buf[3, KA], buf[3, KB]], axis=1), worst)
        for c in chunks:
            fw[VA, c].wait_recv()
            fw[VB, c].wait_recv()
        acc += weighted(jnp.concatenate([buf[3, VA], buf[3, VB]], axis=1), p)
        o_ref[...] = acc[16:] * jnp.tile(pltpu.reciprocal(acc[:8], approx=False), (D // 8, 1))

        @pl.when(jnp.logical_not(jnp.max(worst) <= SAFE_EXP))
        def _():
            def block_scores(slot):
                kt_all = jnp.concatenate([buf[slot, KA], buf[slot, KB]], axis=1)
                return jnp.dot(qb, kt_all, preferred_element_type=f32)

            m = lax.fori_loop(
                1, N_DEV,
                lambda j, m: jnp.maximum(m, jnp.max(block_scores(j), axis=1, keepdims=True)), m0)
            l = lax.fori_loop(
                0, N_DEV,
                lambda j, l: l + jnp.sum(jnp.exp2(block_scores(j) - m), axis=1, keepdims=True),
                jnp.zeros((S, 1), f32))
            inv_l = 1.0 / l

            def add(j, o):
                pj = (jnp.exp2(block_scores(j) - m) * inv_l).astype(bf16)
                vt_all = jnp.concatenate([buf[j, VA], buf[j, VB]], axis=1)
                return o + lax.dot_general(vt_all, pj, NT, preferred_element_type=f32)

            o_ref[...] = lax.fori_loop(0, N_DEV, add, jnp.zeros((D, S), f32))

    out_t = pl.pallas_call(
        body,
        out_shape=jax.ShapeDtypeStruct((D, S), f32),
        in_specs=[pl.BlockSpec(memory_space=pl.ANY)] * 3,
        out_specs=pl.BlockSpec(memory_space=pltpu.VMEM),
        scratch_shapes=[
            pltpu.VMEM((3, D, S), f32),
            pltpu.VMEM((N_DEV, 4, D, HK), bf16),
            pltpu.VMEM((2, NF32, R, HK), f32),
            pltpu.SemaphoreType.DMA((2 * NCH + 1,)),
            pltpu.SemaphoreType.DMA((12 * NCH,)),
            pltpu.SemaphoreType.DMA((12 * NCH,)),
            pltpu.SemaphoreType.REGULAR,
            pltpu.SemaphoreType.DMA((4 * NCH,)),
        ],
        compiler_params=pltpu.CompilerParams(collective_id=0, disable_semaphore_checks=True),
    )(q.T, k.T, v.T)
    return out_t.T
```
